```python
import numpy as np

kernel_name = "dist_moe_cap_ep_n512_d256_e4_h512"

def setup_inputs():
    x = np.random.randn(512, 256).astype(np.float32)
    router_W = np.random.randn(256, 16).astype(np.float32) * 0.1
    scores64 = x.astype(np.float64) @ router_W.astype(np.float64)
    route_idx = np.argsort(-scores64, axis=-1)[:, :1].astype(np.int32)
    expert_W = np.random.randn(16, 256, 512).astype(np.float32) * 0.02
    return {"x": x, "router_W": router_W, "route_idx": route_idx, "expert_W": expert_W}

def reference(x, router_W, route_idx, expert_W):
    counts = np.zeros(16, dtype=np.int64)
    out = np.zeros((512, 512), dtype=np.float32)
    for i in range(512):
        e = int(route_idx[i, 0])
        if counts[e] < 25:
            out[i] = x[i] @ expert_W[e]
            counts[e] += 1
    return out
```

```python
import contextlib

import jax
import jax.numpy as jnp
from jax import lax
from jax.experimental import pallas as pl
from jax.experimental.pallas import tpu as pltpu

N_DEV = 4
N_TOK = 512
D_IN = 256
D_OUT = 512
N_EXP = 16
E_LOC = N_EXP // N_DEV
CAP = 25
SLOTS = 32
LANES = 128
N_BLK = N_TOK // LANES
A, B, C, D = 0, 1, 2, 3

P10 = ((0, 0, 2), (0, 2, 2), (1, 0, 2), (1, 2, 2), (2, 0, 2), (2, 2, 2), (3, 0, 1), (3, 1, 1), (3, 2, 1), (3, 3, 1))

P8 = tuple((e, t, 2) for e in range(4) for t in (0, 2))
P9 = P8[:7] + ((3, 2, 1), (3, 3, 1))

DEFAULT = dict(
    pieces=P10,
    c_via_d=(0, 1, 2, 3),
    a_via_b=(0, 1, 4, 5),
    d_early={},
    c_to_b={},
    diag_order=(4, 5, 0, 1, 6, 2, 7, 8, 3, 9),
    drain_before=3,
    drain_from=6,
    drain_keep=4,
    slots_after=1,
    table_after=2,
    zero_after=3,
    own_after={},
    a_bar=3,
    two=False,
    pdt=jnp.float32,
    scopes=False,
    flags=None,
    wprio=1,
)


def make(**over):
    cfg = dict(DEFAULT, **over)
    pieces = cfg["pieces"]
    n_p = len(pieces)
    rows = [CAP if nt == 2 else (CAP + 1) // 2 for _, _, nt in pieces]
    offs = []
    o = 0
    for _, _, nt in pieces:
        offs.append(o)
        o += SLOTS if nt == 2 else SLOTS // 2
    y_rows = o

    def scope(name):
        on = cfg["scopes"] is True or (cfg["scopes"] and name[0] in cfg["scopes"])
        return jax.named_scope(name) if on else contextlib.nullcontext()

    def body(x_hbm, r_hbm, w_hbm, o_ref, r_v, tok_v, xg, w_v, ybuf, slot_v, tab_v, tab_s,
             r_sem, x_sems, w_sems, t_sem, send_sems, recv_sems, c_ready):
        r_cp = pltpu.make_async_copy(r_hbm, r_v, r_sem)
        r_cp.start()
        w_cps = []
        for p, (e, t0, nt) in enumerate(pieces):
            cols = pl.ds(t0 * LANES, nt * LANES)
            w_cps.append(pltpu.make_async_copy(w_hbm.at[e, :, cols], w_v.at[e, :, cols], w_sems.at[p]))
        w_cps[0].start(priority=cfg["wprio"])

        me = lax.axis_index("i")
        bar = pltpu.get_barrier_semaphore()

        def signal(sem, dev):
            pl.semaphore_signal(sem, inc=1, device_id=(dev,), device_id_type=pl.DeviceIdType.MESH)

        @pl.when(me == A)
        def _():
            signal(bar, C)
            signal(bar, B)
            signal(bar, D)

        @pl.when((me == B) | (me == D))
        def _():
            signal(bar, C)
            signal(bar, A)

        for cp in w_cps[1:]:
            cp.start(priority=cfg["wprio"])

        def msg(at, src, p, dst, k):
            here = pl.ds(offs[p], rows[p])
            return pltpu.make_async_remote_copy(
                ybuf.at[(src - at) % N_DEV, here], ybuf.at[(src - dst) % N_DEV, here],
                send_sems.at[k * n_p + p], recv_sems.at[((src - dst) % N_DEV - 1) * n_p + p],
                device_id=(dst,), device_id_type=pl.DeviceIdType.MESH)

        def arrived(d, p):
            here = ybuf.at[d, pl.ds(offs[p], rows[p])]
            pltpu.make_async_remote_copy(
                here, here, send_sems.at[0], recv_sems.at[(d - 1) * n_p + p],
                device_id=(A,), device_id_type=pl.DeviceIdType.MESH).wait_recv()

        def iota(shape, axis):
            return lax.broadcasted_iota(jnp.int32, shape, axis)

        def prefix_weights():
            tri = (iota((LANES, LANES), 0) <= iota((LANES, LANES), 1)).astype(jnp.float32)
            return jnp.concatenate([tri, jnp.ones((LANES, LANES), jnp.float32)], axis=1).astype(cfg["pdt"])

        def ranks(first, n):
            route = r_v[...] & (N_EXP - 1)
            expert = ((iota((n * N_BLK, LANES), 0) >> 2) + (E_LOC * me + first)) & (N_EXP - 1)
            hot = (jnp.concatenate([route] * n, axis=0) == expert).astype(jnp.float32)
            return jnp.dot(hot.astype(cfg["pdt"]), prefix_weights(), preferred_element_type=jnp.float32)

        def before(pre, j):
            left = iota((SLOTS, LANES), 0).astype(jnp.float32)
            cnt = None
            base = None
            for b in range(N_BLK):
                row = pre[j * N_BLK + b:j * N_BLK + b + 1, :]
                cum = row[:, :LANES] if base is None else row[:, :LANES] + base
                base = row[:, LANES:] if base is None else row[:, LANES:] + base
                m = (cum <= left).astype(jnp.float32)
                cnt = m if cnt is None else cnt + m
            return cnt

        @pl.when(me == C)
        def _():
            pl.semaphore_wait(bar, 3)
            signal(c_ready, B)
            signal(c_ready, D)

        with scope("a_route"):
            r_cp.wait()

        def fetch(e, s, tile, row):
            return pltpu.make_async_copy(x_hbm.at[tile, :, pl.ds(row, 1)], xg.at[e, :, pl.ds(s, 1)], x_sems.at[e])

        def gather(e, tok):
            if cfg["two"]:
                tile, row = tok >> 3, tok & 7
                for s in range(CAP):
                    fetch(e, s, tile[s, 0], row[s, 0]).start()
            else:
                for s in range(CAP):
                    t = tok[s, 0]
                    fetch(e, s, t >> 3, t & 7).start()

        valid = []
        with scope("b_cum"):
            pre = ranks(0, E_LOC)
        for e in range(E_LOC):
            tok = jnp.sum(before(pre, e), axis=1, keepdims=True)
            valid.append((tok < N_TOK) & (iota((SLOTS, 1), 0) < CAP))
            tok = lax.bitcast_convert_type(tok + float(1 << 23), jnp.int32) & (N_TOK - 1)
            if e == 0:
                with scope("c_rows0"):
                    gather(0, tok)
            else:
                tok_v[e] = jnp.broadcast_to(tok, (SLOTS, LANES))

        with scope("c_rows1"):
            @pl.loop(1, E_LOC)
            def _(e):
                gather(e, tok_v[e])

        t_cp = pltpu.make_async_copy(tab_v, tab_s, t_sem)

        def slots():
            local = ((r_v[...] & (N_EXP - 1)) - E_LOC * me) & (N_EXP - 1)
            blocks = [local[b:b + 1, :] for b in range(N_BLK)]
            hot = [(blk == iota((N_EXP, LANES), 0)).astype(jnp.float32) for blk in blocks]
            pre = jnp.dot(jnp.concatenate(hot, axis=0).astype(cfg["pdt"]), prefix_weights(), preferred_element_type=jnp.float32)
            base = None
            for b in range(N_BLK):
                part = pre[b * N_EXP:(b + 1) * N_EXP]
                cum = part[:, :LANES] if base is None else part[:, :LANES] + base
                base = part[:, LANES:] if base is None else part[:, LANES:] + base
                rank = jnp.sum(hot[b] * cum, axis=0, keepdims=True).astype(jnp.int32) - 1
                slot = jnp.where(rank < SLOTS, blocks[b] * SLOTS + rank, -1)
                slot_v[b] = jnp.broadcast_to(slot, (8, LANES))

        def table():
            sub, lane = iota((8, LANES), 0), iota((8, LANES), 1)
            lhs, rhs = [], []
            for b in range(N_BLK):
                slot = slot_v[b]
                tok = lane + b * LANES
                part = jnp.where(sub < N_DEV, (tok >> 3) << 5, (tok & 7) + 1).astype(jnp.float32)
                lhs.append(jnp.where((slot >> 7) == (sub & (N_DEV - 1)), part, 0.0))
                rhs.append(((slot[:1] & (LANES - 1)) == iota((LANES, LANES), 0)).astype(jnp.float32))
            tab = lax.dot_general(jnp.concatenate(lhs, axis=1), jnp.concatenate(rhs, axis=1),
                                  (((1,), (1,)), ((), ())), preferred_element_type=jnp.float32)
            tab = tab[:N_DEV] + tab[N_DEV:] - 1.0
            over = (lane[:N_DEV] & (SLOTS - 1)) >= CAP
            dropped = jnp.max(jnp.max(jnp.where(over, tab, 0.0), axis=0, keepdims=True), axis=1, keepdims=True)
            tab_v[...] = jnp.where(over | (tab < 0.0), dropped, tab).astype(jnp.int32)
            t_cp.start()

        def scatter(d, p):
            e, t0, nt = pieces[p]
            for i in range(rows[p]):
                word = ybuf[d, pl.ds(offs[p] + i, 1), :]
                lo = pltpu.bitcast(word << 16, jnp.float32)
                hi = pltpu.bitcast(word & jnp.uint32(0xFFFF0000), jnp.float32)
                if nt == 2:
                    tok = tab_s[d, e * SLOTS + i]
                    o_ref[pl.ds(tok + 8 * t0, 1), :] = lo
                    o_ref[pl.ds(tok + 8 * (t0 + 1), 1), :] = hi
                else:
                    o_ref[pl.ds(tab_s[d, e * SLOTS + 2 * i] + 8 * t0, 1), :] = lo
                    if 2 * i + 1 < CAP:
                        o_ref[pl.ds(tab_s[d, e * SLOTS + 2 * i + 1] + 8 * t0, 1), :] = hi

        sends = {A: [], B: [], C: [], D: []}

        def send(at, src, p, dst):
            k = {B: {A: 0, C: 1}, D: {A: 0, C: 1}, A: {B: 0, D: 1}, C: {A: 0, B: 1, D: 2}}[at][dst] if src == at \
                else 2 + {A: {B: 0, D: 1}, B: {C: 0}, D: {A: 0, C: 1}}[at][dst]
            msg(at, src, p, dst, k).start()
            sends[at].append((src, p, dst, k))

        relayed = set()
        to_b = set()
        own_done = set()
        xs = {}
        for p, (e, t0, nt) in enumerate(pieces):
            with scope(f"f_w{p}"):
                w_cps[p].wait()
            w = w_v[e, :, t0 * LANES:(t0 + nt) * LANES].astype(jnp.bfloat16)
            if e not in xs:
                with scope(f"e_x{e}"):
                    for i in range(CAP):
                        fetch(e, i, 0, 0).wait()
                xs[e] = jnp.where(valid[e], jnp.concatenate([xg[e, 0], xg[e, 1]], axis=1), 0.0).astype(jnp.bfloat16)
            with scope(f"g_mm{p}"):
                y = jnp.dot(xs[e], w, preferred_element_type=jnp.float32)
                if nt == 2:
                    ybuf[0, offs[p]:offs[p] + SLOTS, :] = pltpu.pack_elementwise(
                        [y[:, :LANES], y[:, LANES:]], packed_dtype=jnp.bfloat16)
                else:
                    ybuf[0, offs[p]:offs[p] + SLOTS // 2, :] = pltpu.bitcast(y.astype(jnp.bfloat16), jnp.uint32)

                @pl.when(me == C)
                def _():
                    if p in cfg["c_via_d"]:
                        send(C, C, p, D)
                        send(C, C, p, B)
                        to_b.add(p)
                    else:
                        send(C, C, p, A)
                        send(C, C, p, D)
                    for q in cfg["c_to_b"].get(p, ()):
                        send(C, C, q, B)
                        to_b.add(q)

                for at in (B, D):
                    @pl.when(me == at)
                    def _():
                        if p == 0:
                            pl.semaphore_wait(bar, 1)
                        send(at, at, p, A)
                        if p == 1:
                            pl.semaphore_wait(c_ready, 1)
                            send(at, at, 0, C)
                        if p >= 1:
                            send(at, at, p, C)
                        if at == D:
                            for q in cfg["d_early"].get(p, ()):
                                with scope(f"h_de{q}"):
                                    arrived((C - D) % N_DEV, q)
                                send(D, C, q, A)
                                relayed.add(q)

                if p >= cfg["a_bar"]:
                    @pl.when(me == A)
                    def _():
                        if p == cfg["a_bar"]:
                            pl.semaphore_wait(bar, 2)
                            for q in range(p):
                                send(A, A, q, B)
                                send(A, A, q, D)
                        send(A, A, p, B)
                        send(A, A, p, D)

            if p == cfg["slots_after"]:
                with scope("d_slots"):
                    slots()
            if p == cfg["table_after"]:
                with scope("d_table"):
                    table()
            if p == cfg["zero_after"]:
                with scope("d_zero"):
                    o_ref[...] = jnp.zeros(o_ref.shape, jnp.float32)
                    t_cp.wait()
            for q in cfg["own_after"].get(p, ()):
                with scope(f"i_own{q}"):
                    scatter(0, q)
                own_done.add(q)

        waited = {A: set(), B: set(), C: set(), D: {((C - D) % N_DEV, q) for q in relayed}}

        with scope("h_relay"):
            @pl.when(me == C)
            def _():
                for p in range(n_p):
                    if p not in to_b:
                        send(C, C, p, B)

            @pl.when(me == D)
            def _():
                for p in cfg["c_via_d"]:
                    if p not in relayed:
                        with scope(f"h_de{p}"):
                            arrived((C - D) % N_DEV, p)
                        waited[D].add(((C - D) % N_DEV, p))
                        send(D, C, p, A)
                for p in range(n_p):
                    if p not in cfg["a_via_b"]:
                        arrived((A - D) % N_DEV, p)
                        waited[D].add(((A - D) % N_DEV, p))
                        send(D, A, p, C)

            @pl.when(me == B)
            def _():
                for p in cfg["a_via_b"]:
                    arrived((A - B) % N_DEV, p)
                    waited[B].add(((A - B) % N_DEV, p))
                    send(B, A, p, C)

        with scope("i_own"):
            for p in range(n_p):
                if p not in own_done:
                    scatter(0, p)

        drained = {at: 0 for at in sends}

        def drain(at, keep=0):
            upto = len(sends[at]) - keep
            for sent in sends[at][drained[at]:upto]:
                msg(at, *sent).wait_send()
            drained[at] = max(drained[at], upto)

        order = [(d, p) for p in range(n_p) for d in (1, 3)] + [(2, p) for p in cfg["diag_order"]]
        for i, (d, p) in enumerate(order):
            if i >= cfg["drain_from"]:
                keep = cfg["drain_keep"] if i < len(order) - cfg["drain_before"] else 0
                if len(sends[A]) - keep > drained[A]:
                    pl.when(me == A)(lambda: drain(A, keep))
            with scope(f"j{d}_{p}"):
                done = [at for at in waited if (d, p) in waited[at]]
                if done:
                    cond = me != done[0]
                    for at in done[1:]:
                        cond = cond & (me != at)
                    pl.when(cond)(lambda: arrived(d, p))
                else:
                    arrived(d, p)
            if d != 2:
                @pl.when(me == A)
                def _():
                    send(A, d, p, N_DEV - d)
            scatter(d, p)

        @pl.loop(0, (me != A).astype(jnp.int32))
        def _(_):
            for at in (B, C, D):
                pl.when(me == at)(lambda: drain(at))

    def fn(x, router_W, route_idx, expert_W):
        hbm = pl.BlockSpec(memory_space=pltpu.HBM)
        out = pl.pallas_call(
            body,
            out_shape=jax.ShapeDtypeStruct((N_TOK * D_OUT // LANES, LANES), jnp.float32),
            in_specs=[hbm, hbm, hbm],
            out_specs=pl.BlockSpec(memory_space=pltpu.VMEM),
            scratch_shapes=[
                pltpu.VMEM((N_BLK, LANES), jnp.int32),
                pltpu.VMEM((E_LOC, SLOTS, LANES), jnp.int32),
                pltpu.VMEM((E_LOC, D_IN // LANES, SLOTS, LANES), jnp.float32),
                pltpu.VMEM((E_LOC, D_IN, D_OUT), jnp.float32),
                pltpu.VMEM((N_DEV, y_rows, LANES), jnp.uint32),
                pltpu.VMEM((N_BLK, 8, LANES), jnp.int32),
                pltpu.VMEM((N_DEV, LANES), jnp.int32),
                pltpu.SMEM((N_DEV, LANES), jnp.int32),
                pltpu.SemaphoreType.DMA,
                pltpu.SemaphoreType.DMA((E_LOC,)),
                pltpu.SemaphoreType.DMA((n_p,)),
                pltpu.SemaphoreType.DMA,
                pltpu.SemaphoreType.DMA((4 * n_p,)),
                pltpu.SemaphoreType.DMA((3 * n_p,)),
                pltpu.SemaphoreType.REGULAR,
            ],
            compiler_params=pltpu.CompilerParams(
                collective_id=0, disable_bounds_checks=True, disable_semaphore_checks=True, flags=cfg["flags"]),
        )(x.reshape(N_TOK // 8, 8, D_IN // LANES, LANES).transpose(0, 2, 1, 3), route_idx.reshape(N_BLK, LANES), expert_W)
        return out.reshape(N_TOK // 8, D_OUT // LANES, 8, LANES).transpose(0, 2, 1, 3).reshape(N_TOK, D_OUT)

    return fn


def pallas_dist_moe_cap_ep_n512_d256_e4_h512_kernel(x, router_W, route_idx, expert_W):
    return make(d_early={7: (0,)}, pdt=jnp.bfloat16)(x, router_W, route_idx, expert_W)
```

```python
import jax
import jax.numpy as jnp
from jax import lax
from jax.experimental import pallas as pl
from jax.experimental.pallas import tpu as pltpu

N_DEV = 4
N_TOK = 512
D_IN = 256
D_OUT = 512
N_EXP = 16
CAP = 25

E_LOC = N_EXP // N_DEV
LANES = 128
SUBLANES = 8
SLOTS = 32
N_BLK = N_TOK // LANES
A, B, C, D = range(N_DEV)

PIECES = tuple((e, (t, t + 1)) for e in (0, 1) for t in (0, 2)) + tuple(
    (e, (t,)) for e in (2, 3) for t in (0, 2, 1, 3)
)
LAST = len(PIECES) - 1


def _layout():
    starts, messages, top = [], [], 0
    for p, (_, tiles) in enumerate(PIECES):
        starts.append(top)
        top += SLOTS if len(tiles) == 2 else SLOTS // 2
        rows = CAP if len(tiles) == 2 else CAP // 2 + p % 2
        if p == LAST:
            messages += [(p, 0, SUBLANES), (p, SUBLANES, rows - SUBLANES)]
        else:
            messages.append((p, 0, rows))
    return tuple(starts), tuple(messages), top


STARTS, MESSAGES, BUF_ROWS = _layout()
N_MSG = len(MESSAGES)

C_TO_A_VIA_D = (0, 2, 3, 4, 5)
A_TO_C_VIA_B = (0, 1, 4, 5, 6, 7)
D_RELAYS_AFTER = 9
A_SENDS_FROM = 2
ACROSS_ORDER = (1, 6, 0, 2, 7, 3, 8, 4, 9, 5, 10, 11, 12)


def _iota(shape, axis):
    return lax.broadcasted_iota(jnp.int32, shape, axis)


def _running_counts(hot):
    square = (LANES, LANES)
    weights = jnp.concatenate(
        [(_iota(square, 0) <= _iota(square, 1)).astype(jnp.float32), jnp.ones(square, jnp.float32)], axis=1
    )
    both = jnp.dot(hot.astype(jnp.bfloat16), weights.astype(jnp.bfloat16), preferred_element_type=jnp.float32)
    return both[:, :LANES], both[:, LANES:]


def _own_tokens(route, me):
    expert = (_iota((E_LOC * N_BLK, LANES), 0) >> 2) + E_LOC * me
    running, total = _running_counts((jnp.concatenate([route] * E_LOC, axis=0) == expert).astype(jnp.float32))
    slot = _iota((SLOTS, LANES), 0).astype(jnp.float32)
    for e in range(E_LOC):
        before = seen = None
        for row in range(e * N_BLK, (e + 1) * N_BLK):
            count, block = running[row : row + 1], total[row : row + 1]
            early = ((count if seen is None else count + seen) <= slot).astype(jnp.float32)
            before = early if before is None else before + early
            seen = block if seen is None else block + seen
        token = jnp.sum(before, axis=1, keepdims=True)
        token = lax.bitcast_convert_type(token + float(1 << 23), jnp.int32) & (N_TOK - 1)
        yield token, slot < jnp.minimum(seen, float(CAP))


def _output_rows(route, me):
    expert = (route - E_LOC * me) & (N_EXP - 1)
    blocks = [expert[b : b + 1] for b in range(N_BLK)]
    hot = [(block == _iota((N_EXP, LANES), 0)).astype(jnp.float32) for block in blocks]
    running, total = _running_counts(jnp.concatenate(hot, axis=0))
    sub, lane = _iota((2 * N_DEV, LANES), 0), _iota((2 * N_DEV, LANES), 1)
    rows, in_slot, seen = [], [], None
    for b in range(N_BLK):
        count, block = running[b * N_EXP : (b + 1) * N_EXP], total[b * N_EXP : (b + 1) * N_EXP]
        rank = jnp.sum(hot[b] * (count if seen is None else count + seen), axis=0, keepdims=True)
        rank = rank.astype(jnp.int32) - 1
        seen = block if seen is None else block + seen
        slot = jnp.where(rank < SLOTS, blocks[b] * SLOTS + rank, -1)
        token = lane + b * LANES
        part = jnp.where(sub < N_DEV, (token >> 3) << 5, (token & 7) + 1).astype(jnp.float32)
        rows.append(jnp.where((slot >> 7) == (sub & (N_DEV - 1)), part, 0.0))
        in_slot.append(((slot & (LANES - 1)) == _iota((LANES, LANES), 0)).astype(jnp.float32))
    table = lax.dot_general(
        jnp.concatenate(rows, axis=1),
        jnp.concatenate(in_slot, axis=1),
        (((1,), (1,)), ((), ())),
        preferred_element_type=jnp.float32,
    )
    table = table[:N_DEV] + table[N_DEV:] - 1.0
    over = (lane[:N_DEV] & (SLOTS - 1)) >= CAP
    dropped = jnp.max(jnp.max(jnp.where(over, table, 0.0), axis=0, keepdims=True), axis=1, keepdims=True)
    return jnp.where(over | (table < 0.0), dropped, table).astype(jnp.int32)


def _kernel(
    x_hbm, route_hbm, w_hbm, out,
    route, tokens, x_rows, w, results, table_vmem, table,
    route_sem, x_sems, w_sems, table_sem, send_sems, recv_sems,
):
    route_copy = pltpu.make_async_copy(route_hbm, route, route_sem)
    route_copy.start()
    w_copies = []
    for p, (e, tiles) in enumerate(PIECES):
        cols = pl.ds(tiles[0] * LANES, len(tiles) * LANES)
        w_copies.append(pltpu.make_async_copy(w_hbm.at[e, :, cols], w.at[e, :, cols], w_sems.at[p]))
    w_copies[0].start(priority=1)

    me = lax.axis_index("i")
    barrier = pltpu.get_barrier_semaphore()

    def signal(chip):
        pl.semaphore_signal(barrier, inc=1, device_id=(chip,), device_id_type=pl.DeviceIdType.MESH)

    signal((me + 1) & (N_DEV - 1))
    signal((me - 1) & (N_DEV - 1))
    pl.when(me == A)(lambda: signal(C))

    for copy in w_copies[1:]:
        copy.start(priority=1)
    out[...] = jnp.zeros(out.shape, out.dtype)

    def fetch_rows(e, token):
        for s in range(CAP):
            t = token[s, 0]
            pltpu.make_async_copy(
                x_hbm.at[t >> 3, :, pl.ds(t & 7, 1)], x_rows.at[e, :, pl.ds(s, 1)], x_sems.at[e]
            ).start()

    route_copy.wait()
    filled = []
    for e, (token, mask) in enumerate(_own_tokens(route[...] & (N_EXP - 1), me)):
        filled.append(mask)
        if e == 0:
            fetch_rows(e, token)
        else:
            tokens[e] = jnp.broadcast_to(token, (SLOTS, LANES))
    pl.loop(1, E_LOC)(lambda e: fetch_rows(e, tokens[e]))

    def rows_of(m):
        p, first, rows = MESSAGES[m]
        return pl.ds(STARTS[p] + first, rows)

    def remote(here, src, m, dst, n):
        there = (src - dst) % N_DEV
        return pltpu.make_async_remote_copy(
            results.at[(src - here) % N_DEV, rows_of(m)],
            results.at[there, rows_of(m)],
            send_sems.at[n],
            recv_sems.at[(there - 1) * N_MSG + m],
            device_id=(dst,),
            device_id_type=pl.DeviceIdType.MESH,
        )

    def wait_for(k, m):
        rows = results.at[k, rows_of(m)]
        pltpu.make_async_remote_copy(
            rows, rows, send_sems.at[0], recv_sems.at[(k - 1) * N_MSG + m],
            device_id=(A,), device_id_type=pl.DeviceIdType.MESH,
        ).wait_recv()

    sent = [[] for _ in range(N_DEV)]
    released = [0] * N_DEV
    received = [[] for _ in range(N_DEV)]

    def send(here, m, dst, src=None):
        sent[here].append((here if src is None else src, m, dst, len(sent[here])))
        remote(here, *sent[here][-1]).start()

    def relay(here, src, m, dst):
        wait_for((src - here) % N_DEV, m)
        received[here].append(((src - here) % N_DEV, m))
        send(here, m, dst, src)

    def release(here, keep=0):
        while released[here] < len(sent[here]) - keep:
            remote(here, *sent[here][released[here]]).wait_send()
            released[here] += 1

    def send_towards_a(m):
        pl.when(me == C)(lambda: send(C, m, D if m in C_TO_A_VIA_D else A))
        pl.when(me == B)(lambda: send(B, m, A))
        pl.when(me == D)(lambda: send(D, m, A))

    def send_to_others(m):
        pl.when(me == C)(lambda: send(C, m, B if m in C_TO_A_VIA_D else D))
        pl.when(me == B)(lambda: send(B, m, C))
        pl.when(me == D)(lambda: send(D, m, C))

    for p, (e, tiles) in enumerate(PIECES):
        if p == 0 or PIECES[p - 1][0] != e:
            fetched = x_rows.at[e, :, pl.ds(0, CAP)]
            pltpu.make_async_copy(fetched, fetched, x_sems.at[e]).wait()
            x = jnp.concatenate([jnp.where(filled[e], x_rows[e, h], 0.0) for h in range(D_IN // LANES)], axis=1)
            x = x.astype(jnp.bfloat16)
        w_copies[p].wait()
        cols = slice(tiles[0] * LANES, (tiles[-1] + 1) * LANES)
        y = jnp.dot(x, w[e, :, cols].astype(jnp.bfloat16), preferred_element_type=jnp.float32)
        if len(tiles) == 2:
            bits = lax.bitcast_convert_type(y.astype(jnp.bfloat16).astype(jnp.float32), jnp.uint32)
            words = (bits[:, :LANES] >> 16) | bits[:, LANES:]
        else:
            if p % 2 == 0:
                odd_slot = y[CAP - 1 : CAP]
            else:
                spare = _iota((SUBLANES, LANES), 0) == CAP % SUBLANES
                y = jnp.concatenate([y[:-SUBLANES], jnp.where(spare, odd_slot, y[-SUBLANES:])], axis=0)
            words = pltpu.bitcast(y.astype(jnp.bfloat16), jnp.uint32)

        mine = [m for m in range(N_MSG) if MESSAGES[m][0] == p]
        for m in mine:
            first = MESSAGES[m][1]
            end = words.shape[0] if m == mine[-1] else first + MESSAGES[m][2]
            results[0, STARTS[p] + first : STARTS[p] + end, :] = words[first:end]
            if m == 0:
                pl.when(me != A)(lambda: pl.semaphore_wait(barrier, jnp.where(me == C, 3, 2)))
            send_towards_a(m)
        for m in mine:
            send_to_others(m)
        if p == D_RELAYS_AFTER:
            pl.when(me == D)(lambda: relay(D, C, C_TO_A_VIA_D[0], A))
        if p >= A_SENDS_FROM:

            @pl.when(me == A)
            def _():
                if p == A_SENDS_FROM:
                    pl.semaphore_wait(barrier, 2)
                for m in range(0 if p == A_SENDS_FROM else mine[0], mine[-1] + 1):
                    send(A, m, B)
                    send(A, m, D)

    @pl.when(me == C)
    def _():
        for m in range(N_MSG):
            if m not in C_TO_A_VIA_D:
                send(C, m, B)

    @pl.when(me == D)
    def _():
        for m in C_TO_A_VIA_D[1:]:
            relay(D, C, m, A)
        for m in range(N_MSG):
            if m not in A_TO_C_VIA_B:
                relay(D, A, m, C)

    @pl.when(me == B)
    def _():
        for m in A_TO_C_VIA_B:
            relay(B, A, m, C)

    table_vmem[...] = _output_rows(route[...] & (N_EXP - 1), me)
    table_copy = pltpu.make_async_copy(table_vmem, table, table_sem)
    table_copy.start()
    table_copy.wait()

    def write_out(k, m):
        p, first, rows = MESSAGES[m]
        e, tiles = PIECES[p]
        for i in range(first, first + rows):
            if len(tiles) == 2:
                places = [(i, tile) for tile in tiles]
            elif 2 * i + 1 < CAP:
                places = [(2 * i, tiles[0]), (2 * i + 1, tiles[0])]
            else:
                places = [(2 * i, tiles[0]), (2 * i, PIECES[p - 1][1][0])]
            word = results[k, pl.ds(STARTS[p] + i, 1), :]
            for (s, tile), bits in zip(places, (word << 16, word & jnp.uint32(0xFFFF0000))):
                row = table[k, e * SLOTS + s] + SUBLANES * tile
                out[pl.ds(row, 1), :] = lax.bitcast_convert_type(bits, jnp.float32)

    order = [(k, m) for m in range(N_MSG) for k in (1, 3)] + [(2, m) for m in ACROSS_ORDER]
    for i, (k, m) in enumerate(order):
        left = len(order) - i
        keep = 0 if left <= 3 else 4 if left <= 5 else 10
        if i >= 6 and released[A] < len(sent[A]) - keep:
            pl.when(me == A)(lambda: release(A, keep))
        pending = True
        for chip in range(N_DEV):
            if (k, m) in received[chip]:
                pending = (me != chip) & pending
        pl.when(pending)(lambda: wait_for(k, m))
        if k != 2:
            pl.when(me == A)(lambda: send(A, m, N_DEV - k, src=k))
        write_out(k, m)
        if k == 3:
            write_out(0, m)

    @pl.loop(0, (me != A).astype(jnp.int32))
    def _(_):
        for chip in (B, C, D):
            pl.when(me == chip)(lambda: release(chip))


def pallas_dist_moe_cap_ep_n512_d256_e4_h512_kernel(
    x: jax.Array,
    router_W: jax.Array,
    route_idx: jax.Array,
    expert_W: jax.Array,
):
    del router_W
    hbm = pl.BlockSpec(memory_space=pltpu.HBM)
    out = pl.pallas_call(
        _kernel,
        out_shape=jax.ShapeDtypeStruct((N_TOK * D_OUT // LANES, LANES), jnp.float32),
        in_specs=[hbm, hbm, hbm],
        out_specs=pl.BlockSpec(memory_space=pltpu.VMEM),
        scratch_shapes=[
            pltpu.VMEM((N_BLK, LANES), jnp.int32),
            pltpu.VMEM((E_LOC, SLOTS, LANES), jnp.int32),
            pltpu.VMEM((E_LOC, D_IN // LANES, SLOTS, LANES), jnp.float32),
            pltpu.VMEM((E_LOC, D_IN, D_OUT), jnp.float32),
            pltpu.VMEM((N_DEV, BUF_ROWS, LANES), jnp.uint32),
            pltpu.VMEM((N_DEV, LANES), jnp.int32),
            pltpu.SMEM((N_DEV, LANES), jnp.int32),
            pltpu.SemaphoreType.DMA,
            pltpu.SemaphoreType.DMA((E_LOC,)),
            pltpu.SemaphoreType.DMA((len(PIECES),)),
            pltpu.SemaphoreType.DMA,
            pltpu.SemaphoreType.DMA((N_DEV * N_MSG,)),
            pltpu.SemaphoreType.DMA(((N_DEV - 1) * N_MSG,)),
        ],
        compiler_params=pltpu.CompilerParams(
            collective_id=0,
            disable_bounds_checks=True,
            disable_semaphore_checks=True,
            flags={"XLA_TPU_FORCE_LP_LLO_SCHEDULER": True},
        ),
    )(
        x.reshape(N_TOK // SUBLANES, SUBLANES, D_IN // LANES, LANES).transpose(0, 2, 1, 3),
        route_idx.reshape(N_BLK, LANES),
        expert_W,
    )
    out = out.reshape(N_TOK // SUBLANES, D_OUT // LANES, SUBLANES, LANES).transpose(0, 2, 1, 3)
    return out.reshape(N_TOK, D_OUT)
```

```python
import jax
import jax.numpy as jnp
from jax import lax
from jax.experimental import pallas as pl
from jax.experimental.pallas import tpu as pltpu

N_DEV = 4
N_TOK = 512
D_IN = 256
D_OUT = 512
N_EXP = 16
CAP = 25

E_LOC = N_EXP // N_DEV
LANES = 128
SUBLANES = 8
SLOTS = 32
N_BLK = N_TOK // LANES
A, B, C, D = range(N_DEV)

PIECES = tuple((e, (t, t + 1)) for e in (0, 1) for t in (0, 2)) + tuple(
    (e, (t,)) for e in (2, 3) for t in (0, 2, 1, 3)
)
LAST = len(PIECES) - 1


def _layout():
    starts, messages, top = [], [], 0
    for p, (_, tiles) in enumerate(PIECES):
        starts.append(top)
        top += SLOTS if len(tiles) == 2 else SLOTS // 2
        rows = CAP if len(tiles) == 2 else CAP // 2 + p % 2
        if p == LAST:
            messages += [(p, 0, SUBLANES), (p, SUBLANES, rows - SUBLANES)]
        else:
            messages.append((p, 0, rows))
    return tuple(starts), tuple(messages), top


STARTS, MESSAGES, BUF_ROWS = _layout()
N_MSG = len(MESSAGES)

C_TO_A_VIA_D = (0, 2, 3, 4, 5)
A_TO_C_VIA_B = (0, 1, 4, 5, 6, 7)
VIA_C = {B: (10, 11, 12), D: (11, 12)}
D_RELAYS_AFTER = 9
ACROSS_ORDER = (1, 6, 0, 2, 7, 3, 8, 9, 4, 10, 11, 5, 12)
A_UNFINISHED = ((5, 0), (8, 4), (33, 14))

HELPS = {A: (B, D, A), B: (C,)}
N_FETCH = E_LOC - 1 + len(HELPS[A])
B_HELPS_AFTER = 2


def _iota(shape, axis):
    return lax.broadcasted_iota(jnp.int32, shape, axis)


def _pack(low, high):
    low, high = (lax.bitcast_convert_type(v.astype(jnp.bfloat16).astype(jnp.float32), jnp.uint32) for v in (low, high))
    return (low >> 16) | high


def _unpack(words):
    return [lax.bitcast_convert_type(v, jnp.float32) for v in (words << 16, words & jnp.uint32(0xFFFF0000))]


def _running_counts(hot):
    square = (LANES, LANES)
    weights = jnp.concatenate(
        [(_iota(square, 0) <= _iota(square, 1)).astype(jnp.float32), jnp.ones(square, jnp.float32)], axis=1
    )
    both = jnp.dot(hot.astype(jnp.bfloat16), weights.astype(jnp.bfloat16), preferred_element_type=jnp.float32)
    return both[:, :LANES], both[:, LANES:]


def _slot_tokens(route, me):
    job = _iota((N_FETCH * N_BLK, LANES), 0) >> 2
    expert = job + E_LOC * me
    for j, chip in enumerate((jnp.where(me == B, HELPS[B][0], HELPS[A][0]), *HELPS[A][1:]), E_LOC - 1):
        expert = jnp.where(job == j, chip * E_LOC + E_LOC - 1, expert)
    running, total = _running_counts((jnp.concatenate([route] * N_FETCH, axis=0) == expert).astype(jnp.float32))
    slot = _iota((SLOTS, LANES), 0).astype(jnp.float32)
    for e in range(N_FETCH):
        before = seen = None
        for row in range(e * N_BLK, (e + 1) * N_BLK):
            count, block = running[row : row + 1], total[row : row + 1]
            early = ((count if seen is None else count + seen) <= slot).astype(jnp.float32)
            before = early if before is None else before + early
            seen = block if seen is None else block + seen
        token = jnp.sum(before, axis=1, keepdims=True)
        token = lax.bitcast_convert_type(token + float(1 << 23), jnp.int32) & (N_TOK - 1)
        yield token, slot < jnp.minimum(seen, float(CAP))


def _output_rows(route, me):
    expert = (route - E_LOC * me) & (N_EXP - 1)
    blocks = [expert[b : b + 1] for b in range(N_BLK)]
    hot = [(block == _iota((N_EXP, LANES), 0)).astype(jnp.float32) for block in blocks]
    running, total = _running_counts(jnp.concatenate(hot, axis=0))
    sub, lane = _iota((2 * N_DEV, LANES), 0), _iota((2 * N_DEV, LANES), 1)
    rows, in_slot, seen = [], [], None
    for b in range(N_BLK):
        count, block = running[b * N_EXP : (b + 1) * N_EXP], total[b * N_EXP : (b + 1) * N_EXP]
        rank = jnp.sum(hot[b] * (count if seen is None else count + seen), axis=0, keepdims=True)
        rank = rank.astype(jnp.int32) - 1
        seen = block if seen is None else block + seen
        slot = jnp.where(rank < SLOTS, blocks[b] * SLOTS + rank, -1)
        token = lane + b * LANES
        part = jnp.where(sub < N_DEV, (token >> 3) << 5, (token & 7) + 1).astype(jnp.float32)
        rows.append(jnp.where((slot >> 7) == (sub & (N_DEV - 1)), part, 0.0))
        in_slot.append(((slot & (LANES - 1)) == _iota((LANES, LANES), 0)).astype(jnp.float32))
    table = lax.dot_general(
        jnp.concatenate(rows, axis=1),
        jnp.concatenate(in_slot, axis=1),
        (((1,), (1,)), ((), ())),
        preferred_element_type=jnp.float32,
    )
    table = table[:N_DEV] + table[N_DEV:] - 1.0
    over = (lane[:N_DEV] & (SLOTS - 1)) >= CAP
    dropped = jnp.max(jnp.max(jnp.where(over, table, 0.0), axis=0, keepdims=True), axis=1, keepdims=True)
    return jnp.where(over | (table < 0.0), dropped, table).astype(jnp.int32)


def _kernel(
    x_hbm, route_hbm, w_hbm, out,
    route, tokens, x_rows, x_out, x_in, w, results, table_vmem, table,
    route_sem, x_sems, x_out_sems, x_in_sem, w_sems, table_sem, send_sems, recv_sems,
):
    route_copy = pltpu.make_async_copy(route_hbm, route, route_sem)
    route_copy.start()
    w_copies = []
    for p, (e, tiles) in enumerate(PIECES):
        cols = pl.ds(tiles[0] * LANES, len(tiles) * LANES)
        w_copies.append(pltpu.make_async_copy(w_hbm.at[e, :, cols], w[p], w_sems.at[p]))
    w_copies[0].start(priority=1)

    me = lax.axis_index("i")
    barrier = pltpu.get_barrier_semaphore()

    def signal(chip):
        pl.semaphore_signal(barrier, inc=1, device_id=(chip,), device_id_type=pl.DeviceIdType.MESH)

    signal((me + 1) & (N_DEV - 1))
    signal((me - 1) & (N_DEV - 1))
    pl.when(me == A)(lambda: signal(C))

    for copy in w_copies[1:]:
        copy.start(priority=1)
    out[...] = jnp.zeros(out.shape, out.dtype)

    def fetch_rows(e, token):
        for s in range(CAP):
            t = token[s, 0]
            pltpu.make_async_copy(
                x_hbm.at[t >> 3, :, pl.ds(t & 7, 1)], x_rows.at[e, :, pl.ds(s, 1)], x_sems.at[e]
            ).start()

    route_copy.wait()
    filled = []
    for e, (token, mask) in enumerate(_slot_tokens(route[...] & (N_EXP - 1), me)):
        filled.append(mask)
        if e == 0:
            fetch_rows(e, token)
        else:
            tokens[e] = jnp.broadcast_to(token, (SLOTS, LANES))
    pl.loop(1, jnp.where(me == A, N_FETCH, jnp.where(me == B, E_LOC, E_LOC - 1)))(lambda e: fetch_rows(e, tokens[e]))

    def fetched_rows(e):
        rows = x_rows.at[e, :, pl.ds(0, CAP)]
        pltpu.make_async_copy(rows, rows, x_sems.at[e]).wait()
        return [jnp.where(filled[e], x_rows[e, h], 0.0) for h in range(D_IN // LANES)]

    def hand_over(j, chip):
        return pltpu.make_async_remote_copy(
            x_out.at[j, pl.ds(0, CAP)], x_in.at[pl.ds(0, CAP)], x_out_sems.at[j], x_in_sem,
            device_id=(chip,), device_id_type=pl.DeviceIdType.MESH,
        )

    @pl.when(me == A)
    def _():
        for j in range(len(HELPS[A]) - 1):
            x_out[j] = _pack(*fetched_rows(E_LOC - 1 + j))

    def rows_of(m):
        p, first, rows = MESSAGES[m]
        return pl.ds(STARTS[p] + first, rows)

    def remote(here, src, m, dst, n):
        there = (src - dst) % N_DEV
        return pltpu.make_async_remote_copy(
            results.at[(src - here) % N_DEV, rows_of(m)],
            results.at[there, rows_of(m)],
            send_sems.at[n],
            recv_sems.at[(there - 1) * N_MSG + m],
            device_id=(dst,),
            device_id_type=pl.DeviceIdType.MESH,
        )

    def wait_for(k, m):
        rows = results.at[k, rows_of(m)]
        pltpu.make_async_remote_copy(
            rows, rows, send_sems.at[0], recv_sems.at[(k - 1) * N_MSG + m],
            device_id=(A,), device_id_type=pl.DeviceIdType.MESH,
        ).wait_recv()

    sent = [[] for _ in range(N_DEV)]
    released = [0] * N_DEV
    received = [[] for _ in range(N_DEV)]

    def send(here, m, dst, src=None):
        sent[here].append((here if src is None else src, m, dst, len(sent[here])))
        remote(here, *sent[here][-1]).start()

    def relay(here, src, m, dst):
        wait_for((src - here) % N_DEV, m)
        received[here].append(((src - here) % N_DEV, m))
        send(here, m, dst, src)

    def release(here, keep=0):
        while released[here] < len(sent[here]) - keep:
            remote(here, *sent[here][released[here]]).wait_send()
            released[here] += 1

    def send_towards_a(m):
        pl.when(me == C)(lambda: send(C, m, D if m in C_TO_A_VIA_D else A))
        pl.when(me == B)(lambda: send(B, m, A))
        pl.when(me == D)(lambda: send(D, m, A))

    def send_to_others(m):
        pl.when(me == C)(lambda: send(C, m, B if m in C_TO_A_VIA_D else D))
        pl.when(me == B)(lambda: send(B, m, C))
        pl.when(me == D)(lambda: send(D, m, C))
        pl.when(me == A)(lambda: send(A, m, B))
        pl.when(me == A)(lambda: send(A, m, D))

    for p, (e, tiles) in enumerate(PIECES):
        if p == 0 or PIECES[p - 1][0] != e:
            if e < E_LOC - 1:
                halves = fetched_rows(e)
            else:

                @pl.when(me == A)
                def _():
                    x_in[...] = _pack(*fetched_rows(N_FETCH - 1))

                pl.when(me != A)(lambda: hand_over(0, A).wait_recv())
                halves = _unpack(jnp.where(_iota((SLOTS, LANES), 0) < CAP, x_in[...], jnp.uint32(0)))
            x = jnp.concatenate(halves, axis=1).astype(jnp.bfloat16)
        w_copies[p].wait()
        y = jnp.dot(x, w[p][...].astype(jnp.bfloat16), preferred_element_type=jnp.float32)
        if len(tiles) == 2:
            words = _pack(y[:, :LANES], y[:, LANES:])
        else:
            if p % 2 == 0:
                odd_slot = y[CAP - 1 : CAP]
            else:
                spare = _iota((SUBLANES, LANES), 0) == CAP % SUBLANES
                y = jnp.concatenate([y[:-SUBLANES], jnp.where(spare, odd_slot, y[-SUBLANES:])], axis=0)
            words = pltpu.bitcast(y.astype(jnp.bfloat16), jnp.uint32)

        mine = [m for m in range(N_MSG) if MESSAGES[m][0] == p]
        for m in mine:
            first = MESSAGES[m][1]
            end = words.shape[0] if m == mine[-1] else first + MESSAGES[m][2]
            results[0, STARTS[p] + first : STARTS[p] + end, :] = words[first:end]
            if m == 0:
                pl.semaphore_wait(barrier, jnp.where(me == C, 3, 2))
            send_towards_a(m)
            if m == 0:
                for j, chip in enumerate(HELPS[A][:-1]):
                    pl.when(me == A)(lambda: hand_over(j, chip).start())
        if p == B_HELPS_AFTER:

            @pl.when(me == B)
            def _():
                x_out[0] = _pack(*fetched_rows(E_LOC - 1))
                hand_over(0, *HELPS[B]).start()

        for m in mine:
            send_to_others(m)
        if p == D_RELAYS_AFTER:
            pl.when(me == D)(lambda: relay(D, C, C_TO_A_VIA_D[0], A))

    @pl.when(me == C)
    def _():
        for m in range(N_MSG):
            if m not in C_TO_A_VIA_D:
                send(C, m, B)
        for src in (B, D):
            for m in VIA_C[src]:
                relay(C, src, m, N_DEV - src)

    @pl.when(me == D)
    def _():
        for m in C_TO_A_VIA_D[1:]:
            relay(D, C, m, A)
        for m in range(N_MSG):
            if m not in A_TO_C_VIA_B:
                relay(D, A, m, C)

    @pl.when(me == B)
    def _():
        for m in A_TO_C_VIA_B:
            relay(B, A, m, C)

    pl.when(me == B)(lambda: hand_over(0, *HELPS[B]).wait_send())
    for j, chip in enumerate(HELPS[A][:-1]):
        pl.when(me == A)(lambda: hand_over(j, chip).wait_send())

    table_vmem[...] = _output_rows(route[...] & (N_EXP - 1), me)
    table_copy = pltpu.make_async_copy(table_vmem, table, table_sem)
    table_copy.start()
    table_copy.wait()

    def write_out(k, m):
        p, first, rows = MESSAGES[m]
        e, tiles = PIECES[p]
        for i in range(first, first + rows):
            if len(tiles) == 2:
                places = [(i, tile) for tile in tiles]
            elif 2 * i + 1 < CAP:
                places = [(2 * i, tiles[0]), (2 * i + 1, tiles[0])]
            else:
                places = [(2 * i, tiles[0]), (2 * i, PIECES[p - 1][1][0])]
            word = results[k, pl.ds(STARTS[p] + i, 1), :]
            for (s, tile), values in zip(places, _unpack(word)):
                row = table[k, e * SLOTS + s] + SUBLANES * tile
                out[pl.ds(row, 1), :] = values

    order = [(k, m) for m in range(N_MSG) for k in (1, 3)] + [(2, m) for m in ACROSS_ORDER]
    for i, (k, m) in enumerate(order):
        keep = [n for to_come, n in A_UNFINISHED if len(order) - i <= to_come]
        if keep and released[A] < len(sent[A]) - keep[0]:
            pl.when(me == A)(lambda: release(A, keep[0]))
        pending = True
        for chip in range(N_DEV):
            if (k, m) in received[chip]:
                pending = (me != chip) & pending
        pl.when(pending)(lambda: wait_for(k, m))
        if k != 2 and m not in VIA_C[k]:
            pl.when(me == A)(lambda: send(A, m, N_DEV - k, src=k))
        write_out(k, m)
        if k == 3:
            write_out(0, m)

    @pl.loop(0, (me != A).astype(jnp.int32))
    def _(_):
        for chip in (B, C, D):
            pl.when(me == chip)(lambda: release(chip))


def pallas_dist_moe_cap_ep_n512_d256_e4_h512_kernel(
    x: jax.Array,
    router_W: jax.Array,
    route_idx: jax.Array,
    expert_W: jax.Array,
):
    del router_W
    hbm = pl.BlockSpec(memory_space=pltpu.HBM)
    out = pl.pallas_call(
        _kernel,
        out_shape=jax.ShapeDtypeStruct((N_TOK * D_OUT // LANES, LANES), jnp.float32),
        in_specs=[hbm, hbm, hbm],
        out_specs=pl.BlockSpec(memory_space=pltpu.VMEM),
        scratch_shapes=[
            pltpu.VMEM((N_BLK, LANES), jnp.int32),
            pltpu.VMEM((N_FETCH, SLOTS, LANES), jnp.int32),
            pltpu.VMEM((N_FETCH, D_IN // LANES, SLOTS, LANES), jnp.float32),
            pltpu.VMEM((len(HELPS[A]) - 1, SLOTS, LANES), jnp.uint32),
            pltpu.VMEM((SLOTS, LANES), jnp.uint32),
            [pltpu.VMEM((D_IN, len(tiles) * LANES), jnp.float32) for _, tiles in PIECES],
            pltpu.VMEM((N_DEV, BUF_ROWS, LANES), jnp.uint32),
            pltpu.VMEM((N_DEV, LANES), jnp.int32),
            pltpu.SMEM((N_DEV, LANES), jnp.int32),
            pltpu.SemaphoreType.DMA,
            pltpu.SemaphoreType.DMA((N_FETCH,)),
            pltpu.SemaphoreType.DMA((len(HELPS[A]) - 1,)),
            pltpu.SemaphoreType.DMA,
            pltpu.SemaphoreType.DMA((len(PIECES),)),
            pltpu.SemaphoreType.DMA,
            pltpu.SemaphoreType.DMA((N_DEV * N_MSG,)),
            pltpu.SemaphoreType.DMA(((N_DEV - 1) * N_MSG,)),
        ],
        compiler_params=pltpu.CompilerParams(
            collective_id=0,
            disable_bounds_checks=True,
            disable_semaphore_checks=True,
            flags={"XLA_TPU_FORCE_LP_LLO_SCHEDULER": True},
        ),
    )(
        x.reshape(N_TOK // SUBLANES, SUBLANES, D_IN // LANES, LANES).transpose(0, 2, 1, 3),
        route_idx.reshape(N_BLK, LANES),
        expert_W,
    )
    out = out.reshape(N_TOK // SUBLANES, D_OUT // LANES, SUBLANES, LANES).transpose(0, 2, 1, 3)
    return out.reshape(N_TOK, D_OUT)
```
